```python
import numpy as np

kernel_name = "dist_ar_i_i_m256_n256"

def setup_inputs():
    return {"x": np.random.randn(1024, 256).astype(np.float32)}

def reference(x: np.ndarray) -> np.ndarray:
    return x.reshape(4, 256, 256).sum(axis=0)
```

```python
import jax
import jax.numpy as jnp
from jax import lax
from jax.experimental import pallas as pl
from jax.experimental.pallas import tpu as pltpu

M = 256
N = 256
HN = N // 2
R = 16
NC = M // R
LOADS = (16, 16, 32, 64, 128)
GROUPS = (8, 4, 2, 1, 1)
MESH = pl.DeviceIdType.MESH


def pallas_dist_ar_i_i_m256_n256_kernel(x):
    NG = len(GROUPS)
    group_of = [g for g, n in enumerate(GROUPS) for _ in range(n)]
    gstart = [sum(GROUPS[:g]) for g in range(NG)]
    lstart = [sum(LOADS[:i]) for i in range(len(LOADS))]

    def body(x_hbm, out_ref, xv, s1, r1, s2, r2, lsem, ssem, rsem1, rsem2, go):
        me = lax.axis_index("i")
        P = (me ^ 1, 3 - me)
        bar = pltpu.get_barrier_semaphore()

        def load(i):
            rows = pl.ds(lstart[i], LOADS[i])
            return pltpu.make_async_copy(x_hbm.at[rows], xv.at[rows], lsem.at[i])

        for i in range(len(LOADS)):
            load(i).start()

        @pl.when(me != 2)
        def _():
            for p in P:
                pl.semaphore_signal(bar, inc=1, device_id=(p,), device_id_type=MESH)

        @pl.when(me % 2 == 1)
        def _():
            pl.semaphore_wait(bar, 1)

        @pl.when(me % 2 == 0)
        def _():
            pl.semaphore_wait(bar, 2)

        @pl.when(me == 2)
        def _():
            for p in P:
                pl.semaphore_signal(go, inc=1, device_id=(p,), device_id_type=MESH)

        def rows(c):
            return pl.ds(c * R, R)

        def cols(h):
            return pl.ds(h * HN, HN)

        def cp1(h, c):
            return pltpu.make_async_remote_copy(
                src_ref=s1.at[h, rows(c)], dst_ref=r1.at[h, rows(c)],
                send_sem=ssem.at[0], recv_sem=rsem1.at[h * NC + c],
                device_id=(P[h],), device_id_type=MESH)

        def cp2(h, c):
            return pltpu.make_async_remote_copy(
                src_ref=s2.at[h, rows(c)], dst_ref=r2.at[h, rows(c)],
                send_sem=ssem.at[1], recv_sem=rsem2.at[h * NG + group_of[c]],
                device_id=(P[1 - h],), device_id_type=MESH)

        for i in range(len(LOADS)):
            load(i).wait()
            c0, c1 = lstart[i] // R, (lstart[i] + LOADS[i]) // R
            rr = pl.ds(lstart[i], LOADS[i])
            for h in range(2):
                s1[h, rr, :] = xv[rr, cols(h)].astype(jnp.bfloat16)

            @pl.when(me != 3)
            def _():
                for c in range(c0, c1):
                    cp1(0, c).start()

            @pl.when(me != 1)
            def _():
                for c in range(c0, c1):
                    cp1(1, c).start()

        for h, who in ((0, 3), (1, 1)):
            @pl.when(me == who)
            def _():
                pl.semaphore_wait(go, 1)
                for c in range(NC):
                    cp1(h, c).start()

        for c in range(NC):
            for h in range(2):
                cp1(h, c).wait_recv()
                s = xv[rows(c), cols(h)] + r1[h, rows(c), :].astype(jnp.float32)
                s2[h, rows(c), :] = s.astype(jnp.bfloat16)
                cp2(h, c).start()
                xv[rows(c), cols(h)] = s

        for g in range(NG):
            rr = pl.ds(gstart[g] * R, GROUPS[g] * R)
            for h in range(2):
                pltpu.make_async_copy(r2.at[h, rr], r2.at[h, rr], rsem2.at[h * NG + g]).wait()
                out_ref[rr, cols(h)] = xv[rr, cols(h)] + r2[h, rr, :].astype(jnp.float32)

        pltpu.make_async_copy(s1, s1, ssem.at[0]).wait()
        pltpu.make_async_copy(s2, s2, ssem.at[1]).wait()

    return pl.pallas_call(
        body,
        out_shape=jax.ShapeDtypeStruct((M, N), jnp.float32),
        in_specs=[pl.BlockSpec(memory_space=pl.ANY)],
        out_specs=pl.BlockSpec(memory_space=pltpu.VMEM),
        scratch_shapes=[
            pltpu.VMEM((M, N), jnp.float32),
            pltpu.VMEM((2, M, HN), jnp.bfloat16),
            pltpu.VMEM((2, M, HN), jnp.bfloat16),
            pltpu.VMEM((2, M, HN), jnp.bfloat16),
            pltpu.VMEM((2, M, HN), jnp.bfloat16),
            pltpu.SemaphoreType.DMA((len(LOADS),)),
            pltpu.SemaphoreType.DMA((2,)),
            pltpu.SemaphoreType.DMA((2 * NC,)),
            pltpu.SemaphoreType.DMA((2 * NG,)),
            pltpu.SemaphoreType.REGULAR,
        ],
        compiler_params=pltpu.CompilerParams(
            collective_id=0,
            disable_semaphore_checks=True,
            disable_bounds_checks=True,
        ),
    )(x)
```

```python
import jax
import jax.numpy as jnp
from jax import lax
from jax.experimental import pallas as pl
from jax.experimental.pallas import tpu as pltpu

M = 256
N = 256
HN = N // 2
BF16 = jnp.bfloat16
F32 = jnp.float32
MESH = pl.DeviceIdType.MESH

R = 2
F = 16
C = 32
NP = M // R
NF = F // R
NC = M // C

SLOTS = (23, 39, 55, 71)

PART = {0: (1, 3), 1: (0, 2), 2: (3, 1), 3: (2, 0)}

LOADS_ALL = ((16, 8), (24, 8))
LOADS_2 = LOADS_ALL + ((32, 16), (48, 16), (64, 16), (80, 16), (96, 32),
                       (128, 64), (192, 64), (0, 16))
LOADS_2_EARLY = 5
LOADS_REST = LOADS_ALL + ((0, 16), (32, 32), (64, 64), (128, 128))

GROUPS_0 = ((0, 128), (128, 88), (216, 32), (248, 8))
GROUPS_REST = ((0, M - C), (M - C, C))


def _group(groups, row):
    return [r0 <= row < r0 + n for r0, n in groups].index(True)


def pallas_dist_ar_i_i_m256_n256_kernel(x: jax.Array):
    def body(x_hbm, out_ref, xv, s1, r1, s2, r2, rf,
             load_sem, send_sem, fine_sem, coarse_sem, sum_sem, go_sem):
        me = lax.axis_index("i")
        bar = pltpu.get_barrier_semaphore()

        def notify(sem, dev):
            pl.semaphore_signal(sem, inc=1, device_id=(dev,), device_id_type=MESH)

        def load(loads, i):
            rows = pl.ds(*loads[i])
            return pltpu.make_async_copy(x_hbm.at[rows], xv.at[rows], load_sem.at[i])

        def start_loads(loads, lo, hi):
            for i in range(lo, hi):
                load(loads, i).start()

        @pl.when((me & 1) == 1)
        def _():
            notify(bar, 2)
            notify(bar, 0)

        start_loads(LOADS_ALL, 0, len(LOADS_ALL))

        def cols(h):
            return pl.ds(h * HN, HN)

        def rcopy(src, dst, ssem, rsem, dev):
            return pltpu.make_async_remote_copy(
                src_ref=src, dst_ref=dst, send_sem=ssem, recv_sem=rsem,
                device_id=(dev,), device_id_type=MESH)

        def fine_piece(h, p, dev):
            rr = pl.ds(p * R, R)
            if p < NF:
                return rcopy(x_hbm.at[rr, cols(h)], rf.at[rr], send_sem.at[2 + h],
                             fine_sem.at[p], dev)
            return rcopy(s1.at[h, rr], r1.at[h, rr], send_sem.at[0], fine_sem.at[p], dev)

        def coarse_rows(h, r0, n, dev):
            rr = pl.ds(r0, n)
            return rcopy(s1.at[h, rr], r1.at[h, rr], send_sem.at[0],
                         coarse_sem.at[h * NC + r0 // C], dev)

        def sum_rows(h, r0, n, dev):
            rr = pl.ds(r0, n)
            g = _group(GROUPS_0, r0) if dev == 0 else 2 * h + _group(GROUPS_REST, r0)
            return rcopy(s2.at[h, rr], r2.at[h, rr], send_sem.at[1], sum_sem.at[g], dev)

        def wait_total(ref, sem):
            pltpu.make_async_copy(ref, ref, sem).wait()

        def cast(loads, i):
            rr = pl.ds(*loads[i])
            for h in range(2):
                s1[h, rr, :] = xv[rr, cols(h)].astype(BF16)

        def coarse_step(h, j, P):
            rr = pl.ds(j * C, C)
            wait_total(r1.at[h, rr], coarse_sem.at[h * NC + j])
            s = xv[rr, cols(h)] + r1[h, rr, :].astype(F32)
            s2[h, rr, :] = s.astype(BF16)
            sum_rows(h, j * C, C, P[1 - h]).start()
            xv[rr, cols(h)] = s

        def finish(h, rr):
            out_ref[rr, cols(h)] = xv[rr, cols(h)] + r2[h, rr, :].astype(F32)

        def finish_rest(order):
            for h, g in order:
                rr = pl.ds(*GROUPS_REST[g])
                wait_total(r2.at[h, rr], sum_sem.at[2 * h + g])
                finish(h, rr)

        @pl.when(me == 2)
        def _():
            P = PART[2]

            def send(r0, n):
                for p in range(r0 // R, (r0 + n) // R):
                    for h in range(2):
                        fine_piece(h, p, P[h]).start()

            start_loads(LOADS_2, len(LOADS_ALL), LOADS_2_EARLY)
            pl.semaphore_wait(bar, 2)
            send(0, F)
            start_loads(LOADS_2, LOADS_2_EARLY, len(LOADS_2))
            notify(go_sem, 1)
            notify(go_sem, 3)
            for i, (r0, n) in enumerate(LOADS_2):
                load(LOADS_2, i).wait()
                if r0 >= F:
                    cast(LOADS_2, i)
                    send(r0, n)
            for j in range(NC):
                for h in range(2):
                    coarse_step(h, j, P)
            for h in range(2):
                rcopy(x_hbm.at[pl.ds(0, F), cols(h)], rf, send_sem.at[2 + h],
                      fine_sem.at[0], P[h]).wait_send()
            wait_total(s1.at[:, pl.ds(F, M - F)], send_sem.at[0])
            finish_rest([(0, 0), (1, 0), (0, 1), (1, 1)])
            wait_total(s2, send_sem.at[1])

        def middle(who):
            P = PART[who]
            hu = P.index(2)
            he = 1 - hu
            start_loads(LOADS_REST, len(LOADS_ALL), len(LOADS_REST))
            pl.semaphore_wait(bar, 1)
            for i, (r0, n) in enumerate(LOADS_REST):
                load(LOADS_REST, i).wait()
                cast(LOADS_REST, i)
                for r in range(r0, r0 + n, C):
                    coarse_rows(he, r, min(n, C), 0).start()
            pl.semaphore_wait(go_sem, 1)
            for j in range(NC):
                coarse_rows(hu, j * C, C, 2).start()
            for p in range(NP):
                rr = pl.ds(p * R, R)
                fine_piece(hu, p, 2).wait_recv()
                got = rf[rr, :] if p < NF else r1[hu, rr, :].astype(F32)
                s2[hu, rr, :] = (xv[rr, cols(hu)] + got).astype(BF16)
                sum_rows(hu, p * R, R, 0).start()
                if p in SLOTS:
                    coarse_step(he, SLOTS.index(p), P)
            rr = pl.ds(0, F)
            xv[rr, cols(hu)] = xv[rr, cols(hu)] + rf[...]
            rr = pl.ds(F, M - F)
            xv[rr, cols(hu)] = xv[rr, cols(hu)] + r1[hu, rr, :].astype(F32)
            for j in range(len(SLOTS), NC):
                coarse_step(he, j, P)
            wait_total(s1, send_sem.at[0])
            finish_rest([(hu, 0), (hu, 1), (he, 0), (he, 1)])
            wait_total(s2, send_sem.at[1])

        @pl.when(me == 1)
        def _():
            middle(1)

        @pl.when(me == 3)
        def _():
            middle(3)

        @pl.when(me == 0)
        def _():
            P = PART[0]
            notify(bar, 1)
            notify(bar, 3)
            start_loads(LOADS_REST, len(LOADS_ALL), len(LOADS_REST))
            for i in range(len(LOADS_REST)):
                load(LOADS_REST, i).wait()
                cast(LOADS_REST, i)
            pl.semaphore_wait(bar, 2)
            for j in range(NC):
                for h in range(2):
                    coarse_rows(h, j * C, C, P[h]).start()
            for j in range(NC):
                for h in range(2):
                    coarse_step(h, j, P)
            wait_total(s1, send_sem.at[0])
            for g in range(len(GROUPS_0)):
                if g == len(GROUPS_0) - 2:
                    wait_total(s2, send_sem.at[1])
                rr = pl.ds(*GROUPS_0[g])
                wait_total(r2.at[:, rr], sum_sem.at[g])
                for h in range(2):
                    finish(h, rr)

    return pl.pallas_call(
        body,
        out_shape=jax.ShapeDtypeStruct((M, N), F32),
        in_specs=[pl.BlockSpec(memory_space=pl.ANY)],
        out_specs=pl.BlockSpec(memory_space=pltpu.VMEM),
        scratch_shapes=[
            pltpu.VMEM((M, N), F32),
            pltpu.VMEM((2, M, HN), BF16),
            pltpu.VMEM((2, M, HN), BF16),
            pltpu.VMEM((2, M, HN), BF16),
            pltpu.VMEM((2, M, HN), BF16),
            pltpu.VMEM((F, HN), F32),
            pltpu.SemaphoreType.DMA((len(LOADS_2),)),
            pltpu.SemaphoreType.DMA((4,)),
            pltpu.SemaphoreType.DMA((NP,)),
            pltpu.SemaphoreType.DMA((2 * NC,)),
            pltpu.SemaphoreType.DMA((4,)),
            pltpu.SemaphoreType.REGULAR,
        ],
        compiler_params=pltpu.CompilerParams(
            collective_id=0,
            disable_semaphore_checks=True,
            disable_bounds_checks=True,
        ),
    )(x)
```
